```python
import numpy as np

kernel_name = "dist_rope_attn_htp_bs_b2_sq512_d1024_hq8_dh128"

def setup_inputs():
    x = np.random.randn(8, 512, 1024).astype(np.float32)
    Wq = np.random.randn(1024, 4096).astype(np.float32) * 0.02
    Wk = np.random.randn(1024, 4096).astype(np.float32) * 0.02
    Wv = np.random.randn(1024, 4096).astype(np.float32) * 0.02
    Wo = np.random.randn(4096, 1024).astype(np.float32) * 0.02
    return {"x": x, "Wq": Wq, "Wk": Wk, "Wv": Wv, "Wo": Wo}

def reference(x, Wq, Wk, Wv, Wo):
    B, Sq, Hq, Dh = 8, 512, 32, 128
    inv = 1.0 / (10000.0 ** (np.arange(0, Dh, 2) / Dh))
    pos = np.arange(Sq)[:, None] * inv[None, :]
    cos = np.repeat(np.cos(pos), 2, axis=-1).astype(np.float32)
    sin = np.repeat(np.sin(pos), 2, axis=-1).astype(np.float32)
    def rot(t):
        t2 = t.reshape(B, Sq, Hq, Dh // 2, 2)
        t_r = np.stack([-t2[..., 1], t2[..., 0]], axis=-1).reshape(B, Sq, Hq, Dh)
        return t * cos[None, :, None, :] + t_r * sin[None, :, None, :]
    Q = rot((x @ Wq).reshape(B, Sq, Hq, Dh))
    K = rot((x @ Wk).reshape(B, Sq, Hq, Dh))
    V = (x @ Wv).reshape(B, Sq, Hq, Dh)
    s = np.einsum('bihd,bjhd->bhij', Q, K).astype(np.float32) * 0.08838834764831843
    s_max = s.max(axis=-1, keepdims=True)
    w = np.exp(s - s_max)
    w = w / w.sum(axis=-1, keepdims=True)
    ctx = np.einsum('bhij,bjhd->bihd', w, V).reshape(B, Sq, Hq * Dh)
    return ctx @ Wo
```

```python
import numpy as np

import jax
import jax.numpy as jnp
from jax import lax
from jax.experimental import pallas as pl
from jax.experimental.pallas import tpu as pltpu

N_DEV = 4
B_LOC = 2
SQ = 512
D = 1024
HQ = 8
DH = 128
SCALE = 0.08838834764831843


def _rope_tables():
    inv = 1.0 / (10000.0 ** (np.arange(0, DH, 2) / DH))
    pos = np.arange(SQ)[:, None] * inv[None, :]
    cos = np.repeat(np.cos(pos), 2, axis=-1).astype(np.float32)
    sin = np.repeat(np.sin(pos), 2, axis=-1).astype(np.float32)
    even = (np.arange(DH) % 2 == 0)[None, :]
    sin_a = np.where(even, -sin, 0.0).astype(np.float32)
    sin_b = np.where(even, 0.0, sin).astype(np.float32)
    return np.stack([cos, sin_a, sin_b], axis=0)


def pallas_dist_rope_attn_htp_bs_b2_sq512_d1024_hq8_dh128_kernel(
    x: jax.Array,
    Wq: jax.Array,
    Wk: jax.Array,
    Wv: jax.Array,
    Wo: jax.Array,
):
    tables = jnp.asarray(_rope_tables())

    def body(x_hbm, wq_hbm, wk_hbm, wv_hbm, wo_hbm, tab_ref, out_ref,
             xf, wf, wqkv, wo_bf, xg, q_s, k_s, v_s, ctx_s,
             send_buf, recv_buf, own_part,
             load_sems, xs_sems, xr_sems, ps_sems, pr_sems):
        me = lax.axis_index("i")
        peers_src = [None, (me + 3) % N_DEV, (me + 1) % N_DEV, (me + 2) % N_DEV]
        peers_dst = [None, (me + 1) % N_DEV, (me + 3) % N_DEV, (me + 2) % N_DEV]

        cp_x = pltpu.make_async_copy(x_hbm, xf, load_sems.at[0])
        cp_x.start()
        cps_w = []
        for j, w_hbm in enumerate([wq_hbm, wk_hbm, wv_hbm, wo_hbm]):
            cp = pltpu.make_async_copy(w_hbm, wf.at[j], load_sems.at[1 + j])
            cp.start()
            cps_w.append(cp)

        cp_x.wait()
        xg[0] = xf[0].astype(jnp.bfloat16)
        xg[7] = xf[1].astype(jnp.bfloat16)

        def x_copy(s, b):
            k = (s - 1) * B_LOC + b
            return pltpu.make_async_remote_copy(
                src_ref=xg.at[7 * b], dst_ref=xg.at[1 + k],
                send_sem=xs_sems.at[k], recv_sem=xr_sems.at[k],
                device_id=(peers_dst[s],), device_id_type=pl.DeviceIdType.MESH)

        x_sends = []
        for s in (1, 2, 3):
            for b in range(B_LOC):
                cp = x_copy(s, b)
                cp.start()
                x_sends.append(cp)

        for j in range(3):
            cps_w[j].wait()
            wqkv[:, j * D:(j + 1) * D] = wf[j].astype(jnp.bfloat16)
        cps_w[3].wait()
        wo_bf[...] = wf[3].astype(jnp.bfloat16)

        cos = tab_ref[0]
        sin_a = tab_ref[1]
        sin_b = tab_ref[2]

        def rope(t, scale):
            r = (t * cos + pltpu.roll(t, DH - 1, 1) * sin_a + pltpu.roll(t, 1, 1) * sin_b)
            return r * scale

        def compute_step(xb):
            qf = jnp.dot(xb, wqkv[:, 0:D], preferred_element_type=jnp.float32)
            for h in range(HQ):
                q_s[:, h * DH:(h + 1) * DH] = rope(qf[:, h * DH:(h + 1) * DH], SCALE).astype(jnp.bfloat16)
            kf = jnp.dot(xb, wqkv[:, D:2 * D], preferred_element_type=jnp.float32)
            for h in range(HQ):
                k_s[:, h * DH:(h + 1) * DH] = rope(kf[:, h * DH:(h + 1) * DH], 1.0).astype(jnp.bfloat16)
            v_s[...] = jnp.dot(xb, wqkv[:, 2 * D:3 * D],
                               preferred_element_type=jnp.float32).astype(jnp.bfloat16)
            for h in range(HQ):
                qh = q_s[:, h * DH:(h + 1) * DH]
                kh = k_s[:, h * DH:(h + 1) * DH]
                vh = v_s[:, h * DH:(h + 1) * DH]
                s = lax.dot_general(qh, kh, (((1,), (1,)), ((), ())),
                                    preferred_element_type=jnp.float32)
                m = jnp.max(s, axis=-1, keepdims=True)
                p = jnp.exp(s - m)
                l = jnp.sum(p, axis=-1, keepdims=True)
                c = jnp.dot(p.astype(jnp.bfloat16), vh, preferred_element_type=jnp.float32)
                ctx_s[:, h * DH:(h + 1) * DH] = (c / l).astype(jnp.bfloat16)
            return jnp.dot(ctx_s[...], wo_bf[...], preferred_element_type=jnp.float32)

        def p_copy(k, dev):
            return pltpu.make_async_remote_copy(
                src_ref=send_buf.at[k], dst_ref=recv_buf.at[k],
                send_sem=ps_sems.at[k], recv_sem=pr_sems.at[k],
                device_id=(dev,), device_id_type=pl.DeviceIdType.MESH)

        def step_body(step, carry):
            is_remote = jnp.logical_and(step >= 1, step <= 6)
            k = jnp.clip(step - 1, 0, 5)

            @pl.when(is_remote)
            def _():
                pltpu.make_async_remote_copy(
                    src_ref=xg.at[0], dst_ref=xg.at[1 + k],
                    send_sem=xs_sems.at[k], recv_sem=xr_sems.at[k],
                    device_id=(me,), device_id_type=pl.DeviceIdType.MESH).wait_recv()

            part = compute_step(xg[step])

            @pl.when(jnp.logical_not(is_remote))
            def _():
                own_part[step // 7] = part

            @pl.when(is_remote)
            def _():
                send_buf[k] = part.astype(jnp.bfloat16)
                slot = (step + 1) // 2
                dev = jnp.where(slot == 1, peers_src[1],
                                jnp.where(slot == 2, peers_src[2], peers_src[3]))
                p_copy(k, dev).start()
            return carry

        lax.fori_loop(0, 8, step_body, 0)

        p_sends = [p_copy(k, me) for k in range(6)]
        for cp in x_sends:
            cp.wait_send()
        for cp in p_sends:
            cp.wait_send()
            cp.wait_recv()

        for b in range(B_LOC):
            acc = own_part[b]
            for s in (1, 2, 3):
                acc = acc + recv_buf[(s - 1) * B_LOC + b].astype(jnp.float32)
            out_ref[b] = acc

    return pl.pallas_call(
        body,
        out_shape=jax.ShapeDtypeStruct((B_LOC, SQ, D), jnp.float32),
        in_specs=[pl.BlockSpec(memory_space=pl.ANY)] * 5
        + [pl.BlockSpec(memory_space=pltpu.VMEM)],
        out_specs=pl.BlockSpec(memory_space=pltpu.VMEM),
        scratch_shapes=[
            pltpu.VMEM((B_LOC, SQ, D), jnp.float32),
            pltpu.VMEM((4, D, D), jnp.float32),
            pltpu.VMEM((D, 3 * D), jnp.bfloat16),
            pltpu.VMEM((D, D), jnp.bfloat16),
            pltpu.VMEM((8, SQ, D), jnp.bfloat16),
            pltpu.VMEM((SQ, D), jnp.bfloat16),
            pltpu.VMEM((SQ, D), jnp.bfloat16),
            pltpu.VMEM((SQ, D), jnp.bfloat16),
            pltpu.VMEM((SQ, D), jnp.bfloat16),
            pltpu.VMEM((6, SQ, D), jnp.bfloat16),
            pltpu.VMEM((6, SQ, D), jnp.bfloat16),
            pltpu.VMEM((B_LOC, SQ, D), jnp.float32),
            pltpu.SemaphoreType.DMA((5,)),
            pltpu.SemaphoreType.DMA((6,)),
            pltpu.SemaphoreType.DMA((6,)),
            pltpu.SemaphoreType.DMA((6,)),
            pltpu.SemaphoreType.DMA((6,)),
        ],
        compiler_params=pltpu.CompilerParams(vmem_limit_bytes=100 * 1024 * 1024),
    )(x, Wq, Wk, Wv, Wo, tables)
```

```python
import math

import jax
import jax.numpy as jnp
from jax import lax
from jax.experimental import pallas as pl
from jax.experimental.pallas import tpu as pltpu

N_DEV = 4
B_LOC = 2
SQ = 512
D = 1024
HQ = 8
DH = 128
SCALE = 0.08838834764831843


def pallas_dist_rope_attn_htp_bs_b2_sq512_d1024_hq8_dh128_kernel(
    x: jax.Array,
    Wq: jax.Array,
    Wk: jax.Array,
    Wv: jax.Array,
    Wo: jax.Array,
):
    def body(x_hbm, wq_hbm, wk_hbm, wv_hbm, wo_hbm, out_ref,
             xf, wf, wqkv, wo_bf, xg, tab, q_s, k_s, v_s, ctx_s,
             send_buf, recv_buf, own_part,
             load_sems, xs_sems, xr_sems, ps_sems, pr_sems):
        me = lax.axis_index("i")
        peers_src = [None, (me + 3) % N_DEV, (me + 1) % N_DEV, (me + 2) % N_DEV]
        peers_dst = [None, (me + 1) % N_DEV, (me + 3) % N_DEV, (me + 2) % N_DEV]

        cp_x = pltpu.make_async_copy(x_hbm, xf, load_sems.at[0])
        cps_w = [pltpu.make_async_copy(w_hbm, wf.at[j], load_sems.at[1 + j])
                 for j, w_hbm in enumerate([wq_hbm, wk_hbm, wv_hbm, wo_hbm])]
        cp_x.start()
        cps_w[0].start()
        cps_w[1].start()

        row = lax.broadcasted_iota(jnp.int32, (SQ, DH), 0).astype(jnp.float32)
        lane = lax.broadcasted_iota(jnp.int32, (SQ, DH), 1)
        pair = (lane // 2).astype(jnp.float32)
        inv = jnp.exp(pair * (-2.0 * math.log(10000.0) / DH))
        ang = row * inv
        cos = jnp.cos(ang)
        sin = jnp.sin(ang)
        even = (lane % 2) == 0
        sin_a = jnp.where(even, -sin, 0.0)
        sin_b = jnp.where(even, 0.0, sin)
        tab[0] = cos
        tab[1] = sin_a
        tab[2] = sin_b
        tab[3] = cos * SCALE
        tab[4] = sin_a * SCALE
        tab[5] = sin_b * SCALE

        cp_x.wait()
        cps_w[2].start()
        xg[0] = xf[0].astype(jnp.bfloat16)
        xg[7] = xf[1].astype(jnp.bfloat16)

        x_sends = []
        for s in (1, 2, 3):
            for b in range(B_LOC):
                k = (s - 1) * B_LOC + b
                cp = pltpu.make_async_remote_copy(
                    src_ref=xg.at[7 * b], dst_ref=xg.at[1 + k],
                    send_sem=xs_sems.at[k], recv_sem=xr_sems.at[k],
                    device_id=(peers_dst[s],), device_id_type=pl.DeviceIdType.MESH)
                if s != 3:
                    cp.start()
                x_sends.append(cp)

        def rope(t, off):
            return (t * tab[off] + pltpu.roll(t, DH - 1, 1) * tab[off + 1]
                    + pltpu.roll(t, 1, 1) * tab[off + 2])

        def p_copy(k, dev):
            return pltpu.make_async_remote_copy(
                src_ref=send_buf.at[k], dst_ref=recv_buf.at[k],
                send_sem=ps_sems.at[k], recv_sem=pr_sems.at[k],
                device_id=(dev,), device_id_type=pl.DeviceIdType.MESH)

        def finish(b):
            acc = own_part[b]
            for s in (1, 2, 3):
                k = (s - 1) * B_LOC + b
                p_copy(k, me).wait_recv()
                acc = acc + recv_buf[k].astype(jnp.float32)
            out_ref[b] = acc

        def step_body(step, carry):
            is_remote = jnp.logical_and(step >= 1, step <= 6)
            first = step == 0
            k = jnp.clip(step - 1, 0, 5)

            @pl.when(is_remote)
            def _():
                pltpu.make_async_remote_copy(
                    src_ref=xg.at[0], dst_ref=xg.at[1 + k],
                    send_sem=xs_sems.at[k], recv_sem=xr_sems.at[k],
                    device_id=(me,), device_id_type=pl.DeviceIdType.MESH).wait_recv()

            @pl.when(step == 1)
            def _():
                x_sends[4].start()
                x_sends[5].start()

            @pl.when(step == 7)
            def _():
                finish(0)

            @pl.when(first)
            def _():
                cps_w[0].wait()
                cps_w[3].start()
                wqkv[:, 0:D] = wf[0].astype(jnp.bfloat16)

            xb = xg[step]
            qf = jnp.dot(xb, wqkv[:, 0:D], preferred_element_type=jnp.float32)
            for h in range(HQ):
                q_s[:, h * DH:(h + 1) * DH] = rope(qf[:, h * DH:(h + 1) * DH], 3).astype(jnp.bfloat16)

            @pl.when(first)
            def _():
                cps_w[1].wait()
                wqkv[:, D:2 * D] = wf[1].astype(jnp.bfloat16)

            kf = jnp.dot(xb, wqkv[:, D:2 * D], preferred_element_type=jnp.float32)
            for h in range(HQ):
                k_s[:, h * DH:(h + 1) * DH] = rope(kf[:, h * DH:(h + 1) * DH], 0).astype(jnp.bfloat16)

            @pl.when(first)
            def _():
                cps_w[2].wait()
                wqkv[:, 2 * D:3 * D] = wf[2].astype(jnp.bfloat16)

            v_s[...] = jnp.dot(xb, wqkv[:, 2 * D:3 * D],
                               preferred_element_type=jnp.float32).astype(jnp.bfloat16)
            for h in range(HQ):
                qh = q_s[:, h * DH:(h + 1) * DH]
                kh = k_s[:, h * DH:(h + 1) * DH]
                vh = v_s[:, h * DH:(h + 1) * DH]
                s = lax.dot_general(qh, kh, (((1,), (1,)), ((), ())),
                                    preferred_element_type=jnp.float32)
                m = jnp.max(s, axis=-1, keepdims=True)
                p = jnp.exp(s - m)
                l = jnp.sum(p, axis=-1, keepdims=True)
                c = jnp.dot(p.astype(jnp.bfloat16), vh, preferred_element_type=jnp.float32)
                ctx_s[:, h * DH:(h + 1) * DH] = (c / l).astype(jnp.bfloat16)

            @pl.when(first)
            def _():
                cps_w[3].wait()
                wo_bf[...] = wf[3].astype(jnp.bfloat16)

            part = jnp.dot(ctx_s[...], wo_bf[...], preferred_element_type=jnp.float32)

            @pl.when(jnp.logical_not(is_remote))
            def _():
                own_part[step // 7] = part

            @pl.when(is_remote)
            def _():
                send_buf[k] = part.astype(jnp.bfloat16)
                slot = (step + 1) // 2
                dev = jnp.where(slot == 1, peers_src[1],
                                jnp.where(slot == 2, peers_src[2], peers_src[3]))
                p_copy(k, dev).start()
            return carry

        lax.fori_loop(0, 8, step_body, 0)

        finish(1)
        for cp in x_sends:
            cp.wait_send()
        for k in range(6):
            p_copy(k, me).wait_send()

    return pl.pallas_call(
        body,
        out_shape=jax.ShapeDtypeStruct((B_LOC, SQ, D), jnp.float32),
        in_specs=[pl.BlockSpec(memory_space=pl.ANY)] * 5,
        out_specs=pl.BlockSpec(memory_space=pltpu.VMEM),
        scratch_shapes=[
            pltpu.VMEM((B_LOC, SQ, D), jnp.float32),
            pltpu.VMEM((4, D, D), jnp.float32),
            pltpu.VMEM((D, 3 * D), jnp.bfloat16),
            pltpu.VMEM((D, D), jnp.bfloat16),
            pltpu.VMEM((8, SQ, D), jnp.bfloat16),
            pltpu.VMEM((6, SQ, DH), jnp.float32),
            pltpu.VMEM((SQ, D), jnp.bfloat16),
            pltpu.VMEM((SQ, D), jnp.bfloat16),
            pltpu.VMEM((SQ, D), jnp.bfloat16),
            pltpu.VMEM((SQ, D), jnp.bfloat16),
            pltpu.VMEM((6, SQ, D), jnp.bfloat16),
            pltpu.VMEM((6, SQ, D), jnp.bfloat16),
            pltpu.VMEM((B_LOC, SQ, D), jnp.float32),
            pltpu.SemaphoreType.DMA((5,)),
            pltpu.SemaphoreType.DMA((6,)),
            pltpu.SemaphoreType.DMA((6,)),
            pltpu.SemaphoreType.DMA((6,)),
            pltpu.SemaphoreType.DMA((6,)),
        ],
        compiler_params=pltpu.CompilerParams(vmem_limit_bytes=100 * 1024 * 1024),
    )(x, Wq, Wk, Wv, Wo)
```
